```python
import numpy as np

kernel_name = "dist_mean_ax0_shard0_i_m1024_n512"

def setup_inputs():
    return {"x": np.random.randn(4096, 512).astype(np.float32)}

def reference(x: np.ndarray) -> np.ndarray:
    return np.mean(x, axis=0, keepdims=True)
```

```python
import jax
import jax.numpy as jnp
from jax import lax
from jax.experimental import pallas as pl
from jax.experimental.pallas import tpu as pltpu

N_DEV = 4
N_CHUNKS = 8


def pallas_dist_mean_ax0_shard0_i_m1024_n512_kernel(
    x: jax.Array,
):
    m, n = x.shape
    rows = m // N_CHUNKS
    inv_count = 1.0 / (m * N_DEV)

    def body(x_hbm, out_ref, buf, comm, load_sems, send_sems, recv_sems):
        my = lax.axis_index("i")

        loads = [
            pltpu.make_async_copy(
                x_hbm.at[pl.ds(c * rows, rows)], buf.at[c], load_sems.at[c]
            )
            for c in range(N_CHUNKS)
        ]
        for ld in loads:
            ld.start()

        barrier = pltpu.get_barrier_semaphore()
        for d in range(1, N_DEV):
            pl.semaphore_signal(
                barrier,
                inc=1,
                device_id=((my + d) % N_DEV,),
                device_id_type=pl.DeviceIdType.MESH,
            )

        acc = jnp.zeros((8, n), jnp.float32)
        for c in range(N_CHUNKS):
            loads[c].wait()
            acc = acc + jnp.sum(buf[c].reshape(rows // 8, 8, n), axis=0)
        comm[0] = jnp.sum(acc, axis=0, keepdims=True)

        pl.semaphore_wait(barrier, N_DEV - 1)

        rdmas = []
        for d in range(1, N_DEV):
            rdma = pltpu.make_async_remote_copy(
                src_ref=comm.at[0],
                dst_ref=comm.at[d],
                send_sem=send_sems.at[d - 1],
                recv_sem=recv_sems.at[d - 1],
                device_id=((my + d) % N_DEV,),
                device_id_type=pl.DeviceIdType.MESH,
            )
            rdma.start()
            rdmas.append(rdma)
        for rdma in rdmas:
            rdma.wait_recv()
        out_ref[...] = (comm[0] + comm[1] + comm[2] + comm[3]) * inv_count
        for rdma in rdmas:
            rdma.wait_send()

    return pl.pallas_call(
        body,
        out_shape=jax.ShapeDtypeStruct((1, n), jnp.float32),
        in_specs=[pl.BlockSpec(memory_space=pl.ANY)],
        out_specs=pl.BlockSpec(memory_space=pltpu.VMEM),
        scratch_shapes=[
            pltpu.VMEM((N_CHUNKS, rows, n), jnp.float32),
            pltpu.VMEM((N_DEV, 1, n), jnp.float32),
            pltpu.SemaphoreType.DMA((N_CHUNKS,)),
            pltpu.SemaphoreType.DMA((N_DEV - 1,)),
            pltpu.SemaphoreType.DMA((N_DEV - 1,)),
        ],
        compiler_params=pltpu.CompilerParams(collective_id=0),
    )(x)
```

```python
import jax
import jax.numpy as jnp
from jax import lax
from jax.experimental import pallas as pl
from jax.experimental.pallas import tpu as pltpu

N_DEV = 4
LANES = 128
SUBLANES = 8

EARLY = 0
LATE = 2

RAW_ROWS = 32
TAIL_CHUNKS = (64, 64, 48, 24, 16, 8)
BIG_CHUNK = 128


def _chunk_sizes(rows):
    head = rows - sum(TAIL_CHUNKS)
    sizes = [BIG_CHUNK] * (head // BIG_CHUNK)
    if head % BIG_CHUNK:
        sizes.append(head % BIG_CHUNK)
    return tuple(sizes) + TAIL_CHUNKS


def _compiler_params():
    try:
        return pltpu.CompilerParams(collective_id=0, disable_semaphore_checks=True)
    except TypeError:
        return pltpu.CompilerParams(collective_id=0)


def pallas_dist_mean_ax0_shard0_i_m1024_n512_kernel(
    x: jax.Array,
):
    m, n = x.shape
    q = n // LANES
    chunks = _chunk_sizes(m - RAW_ROWS)
    offs = [sum(chunks[:c]) for c in range(len(chunks))]
    nc = len(chunks)
    raw_off = m - RAW_ROWS
    inv_count = 1.0 / (m * N_DEV)

    def tree_sum(v):
        parts = [
            v[i * SUBLANES:(i + 1) * SUBLANES] for i in range(v.shape[0] // SUBLANES)
        ]
        while len(parts) > 1:
            nxt = [parts[i] + parts[i + 1] for i in range(0, len(parts) - 1, 2)]
            if len(parts) % 2:
                nxt.append(parts[-1])
            parts = nxt
        return parts[0]

    def fold(a):
        return jnp.sum(a, axis=0, keepdims=True).reshape(q, LANES)

    def body(x_hbm, out_ref, buf, raw, dsend, drecv, comm, load_sems, send_sems, recv_sems):
        my = lax.axis_index("i")

        def peer(d):
            return (my + d) & (N_DEV - 1)

        def load(off, rows, sem):
            return pltpu.make_async_copy(
                x_hbm.at[pl.ds(off, rows)], buf.at[pl.ds(off, rows)], load_sems.at[sem]
            )

        def remote(src, dst, slot, dev):
            return pltpu.make_async_remote_copy(
                src_ref=src,
                dst_ref=dst,
                send_sem=send_sems.at[slot],
                recv_sem=recv_sems.at[slot],
                device_id=(dev,),
                device_id_type=pl.DeviceIdType.MESH,
            )

        def raw_rdma():
            return remote(x_hbm.at[pl.ds(raw_off, RAW_ROWS)], raw, 3, EARLY)

        def diag_rdma():
            return remote(dsend, drecv, 1, peer(2))

        def nbr_rdma(d):
            return remote(comm.at[0], comm.at[d], d - 1, peer(d))

        loads = [load(offs[c], chunks[c], c) for c in range(nc)]
        raw_load = load(raw_off, RAW_ROWS, nc)

        for ld in loads:
            ld.start()
        raw_load.start()
        barrier = pltpu.get_barrier_semaphore()
        for d in (2, 1, 3):
            pl.semaphore_signal(
                barrier,
                inc=1,
                device_id=(peer(d),),
                device_id_type=pl.DeviceIdType.MESH,
            )
        pl.semaphore_wait(barrier, N_DEV - 1)

        @pl.when(my == LATE)
        def _():
            raw_rdma().start()

        acc = None
        for c in range(nc):
            loads[c].wait()
            for s in range(0, chunks[c], 64):
                r = tree_sum(buf[pl.ds(offs[c] + s, min(64, chunks[c] - s)), :])
                acc = r if acc is None else acc + r
        part = fold(acc)
        dsend[...] = part.astype(dsend.dtype)

        @pl.when(my == LATE)
        def _():
            diag_rdma().start()

        raw_load.wait()
        comm[0] = part + fold(tree_sum(buf[pl.ds(raw_off, RAW_ROWS), :]))

        @pl.when(my != LATE)
        def _():
            dsend[...] = comm[0].astype(dsend.dtype)
            diag_rdma().start()

        for d in (1, 3):
            nbr_rdma(d).start()
        diag_rdma().wait_send()
        for d in (1, 3):
            nbr_rdma(d).wait_send()

        @pl.when(my == LATE)
        def _():
            raw_rdma().wait_send()

        for d in (1, 3):
            nbr_rdma(d).wait_recv()
        comm[2] = comm[0] + comm[1] + comm[3]

        @pl.when(my == EARLY)
        def _():
            raw_rdma().wait_recv()
            comm[2] = comm[2] + fold(tree_sum(raw[...]))

        rest = comm[2]
        diag_rdma().wait_recv()
        total = rest + drecv[...].astype(jnp.float32)
        out_ref[...] = (total * inv_count).reshape(1, n)

    return pl.pallas_call(
        body,
        out_shape=jax.ShapeDtypeStruct((1, n), jnp.float32),
        in_specs=[pl.BlockSpec(memory_space=pl.ANY)],
        out_specs=pl.BlockSpec(memory_space=pltpu.VMEM),
        scratch_shapes=[
            pltpu.VMEM((m, n), jnp.float32),
            pltpu.VMEM((RAW_ROWS, n), jnp.float32),
            pltpu.VMEM((q, LANES), jnp.bfloat16),
            pltpu.VMEM((q, LANES), jnp.bfloat16),
            pltpu.VMEM((N_DEV, q, LANES), jnp.float32),
            pltpu.SemaphoreType.DMA((nc + 1,)),
            pltpu.SemaphoreType.DMA((N_DEV,)),
            pltpu.SemaphoreType.DMA((N_DEV,)),
        ],
        compiler_params=_compiler_params(),
    )(x)
```

```python
import jax
import jax.numpy as jnp
from jax import lax
from jax.experimental import pallas as pl
from jax.experimental.pallas import tpu as pltpu

N_DEV = 4
LANES = 128
SUBLANES = 8

EARLY = 0
LATE = 2

RAW_ROWS = 32
TAIL_CHUNKS = (64, 64, 48, 24, 16, 8)
BIG_CHUNK = 128


def _chunk_sizes(rows):
    head = rows - sum(TAIL_CHUNKS)
    sizes = [BIG_CHUNK] * (head // BIG_CHUNK)
    if head % BIG_CHUNK:
        sizes.append(head % BIG_CHUNK)
    return tuple(sizes) + TAIL_CHUNKS


def _compiler_params():
    try:
        return pltpu.CompilerParams(collective_id=0, disable_semaphore_checks=True)
    except TypeError:
        return pltpu.CompilerParams(collective_id=0)


def pallas_dist_mean_ax0_shard0_i_m1024_n512_kernel(
    x: jax.Array,
):
    m, n = x.shape
    q = n // LANES
    chunks = _chunk_sizes(m - RAW_ROWS)
    offs = [sum(chunks[:c]) for c in range(len(chunks))]
    nc = len(chunks)
    raw_off = m - RAW_ROWS
    inv_count = 1.0 / (m * N_DEV)

    def tree_sum(v):
        parts = [
            v[i * SUBLANES:(i + 1) * SUBLANES] for i in range(v.shape[0] // SUBLANES)
        ]
        while len(parts) > 1:
            nxt = [parts[i] + parts[i + 1] for i in range(0, len(parts) - 1, 2)]
            if len(parts) % 2:
                nxt.append(parts[-1])
            parts = nxt
        return parts[0]

    def fold(a):
        return jnp.sum(a, axis=0, keepdims=True).reshape(q, LANES)

    def body(x_hbm, out_ref, buf, raw, dsend, drecv, comm, load_sems, send_sems, recv_sems):
        my = lax.axis_index("i")

        def peer(d):
            return (my + d) & (N_DEV - 1)

        def load(off, rows, sem):
            return pltpu.make_async_copy(
                x_hbm.at[pl.ds(off, rows)], buf.at[pl.ds(off, rows)], load_sems.at[sem]
            )

        def remote(src, dst, slot, dev):
            return pltpu.make_async_remote_copy(
                src_ref=src,
                dst_ref=dst,
                send_sem=send_sems.at[slot],
                recv_sem=recv_sems.at[slot],
                device_id=(dev,),
                device_id_type=pl.DeviceIdType.MESH,
            )

        def raw_rdma():
            return remote(x_hbm.at[pl.ds(raw_off, RAW_ROWS)], raw, 3, EARLY)

        def diag_rdma():
            return remote(dsend, drecv, 1, peer(2))

        def nbr_rdma(d):
            return remote(comm.at[0], comm.at[d], d - 1, peer(d))

        loads = [load(offs[c], chunks[c], c) for c in range(nc)]
        raw_load = load(raw_off, RAW_ROWS, nc)

        for ld in loads:
            ld.start()
        raw_load.start()
        barrier = pltpu.get_barrier_semaphore()
        for d in (2, 1, 3):
            pl.semaphore_signal(
                barrier,
                inc=1,
                device_id=(peer(d),),
                device_id_type=pl.DeviceIdType.MESH,
            )
        pl.semaphore_wait(barrier, N_DEV - 1)

        @pl.when(my == LATE)
        def _():
            raw_rdma().start()

        acc = None
        for c in range(nc - 1):
            loads[c].wait()
            for s in range(0, chunks[c], 64):
                r = tree_sum(buf[pl.ds(offs[c] + s, min(64, chunks[c] - s)), :])
                acc = r if acc is None else acc + r
        head = fold(acc)
        loads[nc - 1].wait()
        rows = [buf[pl.ds(offs[nc - 1] + r, 1), :] for r in range(chunks[nc - 1])]
        while len(rows) > 1:
            rows = [rows[i] + rows[i + 1] for i in range(0, len(rows), 2)]
        part = head + rows[0].reshape(q, LANES)
        dsend[...] = part.astype(dsend.dtype)

        @pl.when(my == LATE)
        def _():
            diag_rdma().start()

        raw_load.wait()
        comm[0] = part + fold(tree_sum(buf[pl.ds(raw_off, RAW_ROWS), :]))

        @pl.when(my != LATE)
        def _():
            dsend[...] = comm[0].astype(dsend.dtype)
            diag_rdma().start()

        for d in (1, 3):
            nbr_rdma(d).start()
        diag_rdma().wait_send()
        for d in (1, 3):
            nbr_rdma(d).wait_send()

        @pl.when(my == LATE)
        def _():
            raw_rdma().wait_send()

        for d in (1, 3):
            nbr_rdma(d).wait_recv()
        comm[2] = comm[0] + comm[1] + comm[3]

        @pl.when(my == EARLY)
        def _():
            raw_rdma().wait_recv()
            comm[2] = comm[2] + fold(tree_sum(raw[...]))

        rest = comm[2]
        diag_rdma().wait_recv()
        total = rest + drecv[...].astype(jnp.float32)
        out_ref[...] = total * inv_count

    out = pl.pallas_call(
        body,
        out_shape=jax.ShapeDtypeStruct((q, LANES), jnp.float32),
        in_specs=[pl.BlockSpec(memory_space=pl.ANY)],
        out_specs=pl.BlockSpec(memory_space=pltpu.VMEM),
        scratch_shapes=[
            pltpu.VMEM((m, n), jnp.float32),
            pltpu.VMEM((RAW_ROWS, n), jnp.float32),
            pltpu.VMEM((q, LANES), jnp.bfloat16),
            pltpu.VMEM((q, LANES), jnp.bfloat16),
            pltpu.VMEM((N_DEV, q, LANES), jnp.float32),
            pltpu.SemaphoreType.DMA((nc + 1,)),
            pltpu.SemaphoreType.DMA((N_DEV,)),
            pltpu.SemaphoreType.DMA((N_DEV,)),
        ],
        compiler_params=_compiler_params(),
    )(x)
    return out.reshape(1, n)
```
